```python
import numpy as np

kernel_name = "dist_moe_cap_ep_tokshard_n2048_d512_e8_h1024"

def setup_inputs():
    x = np.random.randn(8192, 512).astype(np.float32)
    router_W = np.random.randn(512, 32).astype(np.float32) * 0.1
    scores64 = x.astype(np.float64) @ router_W.astype(np.float64)
    route_idx = np.argsort(-scores64, axis=-1)[:, :1].astype(np.int32)
    expert_W = np.random.randn(32, 512, 1024).astype(np.float32) * 0.02
    return {"x": x, "router_W": router_W, "route_idx": route_idx, "expert_W": expert_W}

def reference(x, router_W, route_idx, expert_W):
    counts = np.zeros(32, dtype=np.int64)
    out = np.zeros((8192, 1024), dtype=np.float32)
    for i in range(8192):
        e = int(route_idx[i, 0])
        if counts[e] < 204:
            out[i] = x[i] @ expert_W[e]
            counts[e] += 1
    return out
```

```python
import jax
import jax.numpy as jnp
from jax import lax
from jax.experimental import pallas as pl
from jax.experimental.pallas import tpu as pltpu

NDEV = 4
T = 2048
D = 512
H = 1024
EL = 8
E = NDEV * EL
CAP = 204
CAPP = 208
XR = D // 256
YR = H // 256
SPARE = E * CAPP
TR = T // 128
XCH = 512
OCH = 256
MESH = pl.DeviceIdType.MESH


def _pack(lo, hi):
    w = pltpu.pack_elementwise([lo, hi], packed_dtype=jnp.bfloat16)
    return pltpu.bitcast(w, jnp.uint32)


def _unpack(w, i):
    return pltpu.unpack_elementwise(
        w, index=i, packed_dtype=jnp.bfloat16, unpacked_dtype=jnp.float32)


def _body(idx_ref, x_hbm, w_hbm, out_hbm,
          xf, xp, sbuf, ebuf, wf, ybuf, rbuf, tbuf, obuf,
          cum_all, slot_v, slot2_v, tab_v, slot_s, slot2_s, tab_s,
          xsem, wsem, osem, ssem, c_send, c_recv,
          d_send, d_recv, r_send, r_recv):
    me = lax.axis_index("i")

    def x_copy(c):
        rows = pl.ds(c * XCH, XCH)
        return pltpu.make_async_copy(x_hbm.at[rows], xf.at[rows], xsem.at[c])

    def w_copy(j):
        return pltpu.make_async_copy(w_hbm.at[j], wf.at[j], wsem.at[j])

    for c in range(T // XCH):
        x_copy(c).start()

    barrier = pltpu.get_barrier_semaphore()
    for k in range(1, NDEV):
        pl.semaphore_signal(barrier, 1, device_id=((me + k) % NDEV,), device_id_type=MESH)

    for j in range(EL):
        w_copy(j).start()

    idx = idx_ref[...]
    hot = [idx == e for e in range(E)]
    row = lax.broadcasted_iota(jnp.int32, (128, 128), 0)
    col = lax.broadcasted_iota(jnp.int32, (128, 128), 1)
    upper = jnp.where(row < col, 1.0, 0.0).astype(jnp.bfloat16)
    ones = jnp.ones((128, 128), jnp.bfloat16)
    lower = jnp.where((row > col) & (row // TR == col // TR), 1.0, 0.0).astype(jnp.bfloat16)
    lane = lax.broadcasted_iota(jnp.int32, (TR, 128), 1)
    rank = jnp.zeros((TR, 128), jnp.float32)
    cum = jnp.zeros((TR, 128), jnp.float32)
    per = 128 // TR
    for g in range(E // per):
        m = jnp.concatenate(
            [jnp.where(hot[g * per + k], 1.0, 0.0) for k in range(per)], axis=0
        ).astype(jnp.bfloat16)
        inrow = jnp.dot(m, upper, preferred_element_type=jnp.float32)
        rowtot = jnp.dot(m, ones, preferred_element_type=jnp.float32)
        before = jnp.dot(lower, rowtot.astype(jnp.bfloat16), preferred_element_type=jnp.float32)
        pre = inrow + before
        incl = before + rowtot
        for k in range(per):
            e = g * per + k
            rank = jnp.where(hot[e], pre[k * TR:(k + 1) * TR], rank)
            cum = jnp.where(lane == e, incl[k * TR:(k + 1) * TR], cum)
    rank = rank.astype(jnp.int32)
    valid = (idx >= 0) & (idx < E) & (rank < CAP)
    slot = jnp.where(valid, idx * CAPP + rank, SPARE)
    slot_v[...] = slot * XR
    slot_cp = pltpu.make_async_copy(slot_v, slot_s, ssem.at[0])
    slot_cp.start()
    cum_all[me] = cum.astype(jnp.int32)

    ebuf[...] = jnp.zeros(ebuf.shape, jnp.uint32)
    rbuf[pl.ds(SPARE * YR, 8), :] = jnp.zeros((8, 128), jnp.uint32)

    pl.semaphore_wait(barrier, NDEV - 1)

    def c_copy(k):
        return pltpu.make_async_remote_copy(
            cum_all.at[me], cum_all.at[me], c_send.at[k], c_recv.at[k],
            device_id=((me + k) % NDEV,), device_id_type=MESH)

    for k in range(1, NDEV):
        c_copy(k).start()

    slot_cp.wait()
    for c in range(T // XCH):
        x_copy(c).wait()

        def pack_rows(b, _):
            r0 = pl.multiple_of(c * XCH + b * 64, 64)
            for q in range(XR):
                lo = xf[pl.ds(r0, 64), q * 128:(q + 1) * 128]
                hi = xf[pl.ds(r0, 64), (q + XR) * 128:(q + XR + 1) * 128]
                xp[pl.ds(r0 * XR + q, 64, stride=XR), :] = _pack(lo, hi)
        lax.fori_loop(0, XCH // 64, pack_rows, None)

        def sort_rows(b, _):
            r = c * (XCH // 128) + b
            for l in range(128):
                sbuf[pl.ds(slot_s[r, l], XR), :] = xp[pl.ds((r * 128 + l) * XR, XR), :]
        lax.fori_loop(0, XCH // 128, sort_rows, None)

    for k in range(1, NDEV):
        c_copy(k).wait_recv()
    srow = lax.broadcasted_iota(jnp.int32, (8, 128), 0)
    tab = jnp.zeros((8, 128), jnp.int32)
    base = jnp.zeros((1, 128), jnp.int32)
    for s in range(NDEV):
        cnt = cum_all[s, TR - 1:TR, :]
        kept = jnp.clip(CAP - base, 0, cnt)
        tab = jnp.where(srow == s, jnp.minimum(base, CAP), tab)
        tab = jnp.where(srow == NDEV + s, kept, tab)
        base = base + cnt
    tab_v[...] = tab
    tab_cp = pltpu.make_async_copy(tab_v, tab_s, ssem.at[1])
    tab_cp.start()
    tab_cp.wait()

    def d_copy(src, dst, j, k):
        e = dst * EL + j
        n = tab_s[NDEV + src, e] * XR
        s_ref = sbuf.at[pl.ds(e * (CAPP * XR), n)]
        d_ref = ebuf.at[j, pl.ds(tab_s[src, e] * XR, n)]
        if k == 0:
            return n, pltpu.make_async_copy(s_ref, d_ref, d_recv.at[j, 0])
        return n, pltpu.make_async_remote_copy(
            s_ref, d_ref, d_send.at[j, k], d_recv.at[j, k],
            device_id=(dst,), device_id_type=MESH)

    def dispatch(j, _):
        for k in (2, 1, 3, 0):
            n, cp = d_copy(me, (me + k) % NDEV, j, k)
            pl.when(n > 0)(cp.start)
    lax.fori_loop(0, EL, dispatch, None)

    lim = jnp.zeros((TR, 128), jnp.int32)
    for e in range(E):
        lim = jnp.where(hot[e], tab_s[NDEV + me, e], lim)
    slot2_v[...] = jnp.where(rank < lim, slot, SPARE) * YR
    slot2_cp = pltpu.make_async_copy(slot2_v, slot2_s, ssem.at[2])
    slot2_cp.start()

    def r_copy(own, dst, j, k):
        e = own * EL + j
        n = tab_s[NDEV + dst, e] * YR
        s_ref = ybuf.at[j, pl.ds(tab_s[dst, e] * YR, n)]
        d_ref = rbuf.at[pl.ds(e * (CAPP * YR), n)]
        if k == 0:
            return n, pltpu.make_async_copy(s_ref, d_ref, r_recv.at[j, 0])
        return n, pltpu.make_async_remote_copy(
            s_ref, d_ref, r_send.at[j, k], r_recv.at[j, k],
            device_id=(dst,), device_id_type=MESH)

    def expert(j, _):
        w_copy(j).wait()
        for k in range(NDEV):
            n, cp = d_copy((me - k) % NDEV, me, j, k)
            pl.when(n > 0)(cp.wait if k == 0 else cp.wait_recv)
        a = [ebuf[j, pl.ds(q, CAPP, stride=XR), :] for q in range(XR)]
        lhs = jnp.concatenate(
            [_unpack(a[q], i).astype(jnp.bfloat16) for i in range(2) for q in range(XR)],
            axis=1)
        for q in range(YR):
            lo = jnp.dot(lhs, wf[j, :, q * 128:(q + 1) * 128].astype(jnp.bfloat16),
                         preferred_element_type=jnp.float32)
            hi = jnp.dot(lhs, wf[j, :, (q + YR) * 128:(q + YR + 1) * 128].astype(jnp.bfloat16),
                         preferred_element_type=jnp.float32)
            ybuf[j, pl.ds(q, CAPP, stride=YR), :] = _pack(lo, hi)
        for k in (2, 1, 3, 0):
            n, cp = r_copy(me, (me + k) % NDEV, j, k)
            pl.when(n > 0)(cp.start)
    lax.fori_loop(0, EL, expert, None)

    def gather(j, _):
        for k in range(NDEV):
            n, cp = r_copy((me - k) % NDEV, me, j, k)
            pl.when(n > 0)(cp.wait if k == 0 else cp.wait_recv)
    lax.fori_loop(0, EL, gather, None)
    slot2_cp.wait()

    def o_copy(c):
        rows = pl.ds(pl.multiple_of(c * OCH, OCH), OCH)
        return pltpu.make_async_copy(obuf.at[rows], out_hbm.at[rows], osem.at[c])

    def combine(c, _):
        def unsort_rows(b, _):
            r = c * (OCH // 128) + b
            for l in range(128):
                tbuf[pl.ds((r * 128 + l) * YR, YR), :] = rbuf[pl.ds(slot2_s[r, l], YR), :]
        lax.fori_loop(0, OCH // 128, unsort_rows, None)

        def unpack_rows(b, _):
            r0 = pl.multiple_of(c * OCH + b * 32, 32)
            for q in range(YR):
                w = tbuf[pl.ds(r0 * YR + q, 32, stride=YR), :]
                obuf[pl.ds(r0, 32), q * 128:(q + 1) * 128] = _unpack(w, 0)
                obuf[pl.ds(r0, 32), (q + YR) * 128:(q + YR + 1) * 128] = _unpack(w, 1)
        lax.fori_loop(0, OCH // 32, unpack_rows, None)
        o_copy(c).start()
    lax.fori_loop(0, T // OCH, combine, None)

    for k in range(1, NDEV):
        c_copy(k).wait_send()

    def drain(j, _):
        for k in range(1, NDEV):
            n, cp = d_copy(me, (me + k) % NDEV, j, k)
            pl.when(n > 0)(cp.wait_send)
            n, cp = r_copy(me, (me + k) % NDEV, j, k)
            pl.when(n > 0)(cp.wait_send)
    lax.fori_loop(0, EL, drain, None)

    def drain_out(c, _):
        o_copy(c).wait()
    lax.fori_loop(0, T // OCH, drain_out, None)


def pallas_dist_moe_cap_ep_tokshard_n2048_d512_e8_h1024_kernel(
    x: jax.Array,
    router_W: jax.Array,
    route_idx: jax.Array,
    expert_W: jax.Array,
):
    del router_W
    u32, i32, f32 = jnp.uint32, jnp.int32, jnp.float32
    dma = pltpu.SemaphoreType.DMA
    return pl.pallas_call(
        _body,
        out_shape=jax.ShapeDtypeStruct((T, H), f32),
        in_specs=[
            pl.BlockSpec(memory_space=pltpu.VMEM),
            pl.BlockSpec(memory_space=pl.ANY),
            pl.BlockSpec(memory_space=pl.ANY),
        ],
        out_specs=pl.BlockSpec(memory_space=pl.ANY),
        scratch_shapes=[
            pltpu.VMEM((T, D), f32),
            pltpu.VMEM((T * XR, 128), u32),
            pltpu.VMEM((SPARE * XR + 8, 128), u32),
            pltpu.VMEM((EL, CAPP * XR, 128), u32),
            pltpu.VMEM((EL, D, H), f32),
            pltpu.VMEM((EL, CAPP * YR, 128), u32),
            pltpu.VMEM((SPARE * YR + 8, 128), u32),
            pltpu.VMEM((T * YR, 128), u32),
            pltpu.VMEM((T, H), f32),
            pltpu.VMEM((NDEV, TR, 128), i32),
            pltpu.VMEM((TR, 128), i32),
            pltpu.VMEM((TR, 128), i32),
            pltpu.VMEM((8, 128), i32),
            pltpu.SMEM((TR, 128), i32),
            pltpu.SMEM((TR, 128), i32),
            pltpu.SMEM((8, 128), i32),
            dma((T // XCH,)), dma((EL,)), dma((T // OCH,)), dma((3,)),
            dma((NDEV,)), dma((NDEV,)),
            dma((EL, NDEV)), dma((EL, NDEV)), dma((EL, NDEV)), dma((EL, NDEV)),
        ],
        compiler_params=pltpu.CompilerParams(
            collective_id=0, vmem_limit_bytes=100 * 2**20),
    )(route_idx.reshape(TR, 128), x, expert_W)
```

```python
import jax
import jax.numpy as jnp
from jax import lax
from jax.experimental import pallas as pl
from jax.experimental.pallas import tpu as pltpu

NDEV = 4
T = 2048
D = 512
H = 1024
EL = 8
E = NDEV * EL
CAP = 204
CAPP = 208
XR = D // 256
YR = H // 256
SPARE = E * CAPP
TR = T // 128
NCH = 8
XCH = T // NCH
CR = TR // NCH
AHEAD = 3
BLIND = 3
EARLY = 3
BIAS_A = -200
BIAS_B = 300
HALF = EL // 2
MESH = pl.DeviceIdType.MESH
assert BLIND * CR < 8 and BLIND <= EARLY


def _pack(lo, hi):
    lo, hi = (lax.bitcast_convert_type(
        v.astype(jnp.bfloat16).astype(jnp.float32), jnp.uint32) for v in (lo, hi))
    return (lo >> 16) | hi


def _unpack(w, i):
    return lax.bitcast_convert_type(w << 16 if i == 0 else w >> 16 << 16, jnp.float32)


def _body(idx_hbm, x_hbm, w_hbm, out_ref,
          xf, xp, sbuf, ebuf, wf, ybuf, rbuf, xfwd, yfwd,
          idx_v, cnt_all, slot_v, tab_v, slot_s, tab_s, inv_s, share_s,
          xsem, lsem, c_recv, x_send, y_send,
          d_recv, f_recv, g_recv, near_recv, diag_recv):
    me = lax.axis_index("i")
    up, down, diag = (me + 1) % NDEV, (me + 3) % NDEV, (me + 2) % NDEV

    def x_copy(c):
        rows = pl.ds(c * XCH, XCH)
        return pltpu.make_async_copy(x_hbm.at[rows], xf.at[rows], xsem.at[c])

    def w_copy(j):
        return pltpu.make_async_copy(w_hbm.at[j], wf.at[j], xsem.at[j])

    def remote(src, dst, send_sem, recv_sem, to):
        return pltpu.make_async_remote_copy(
            src, dst, send_sem, recv_sem, device_id=(to,), device_id_type=MESH)

    def wait_rows(buf, rows, sem):
        @pl.when(rows > 0)
        def _():
            span = buf.at[pl.ds(0, rows)]
            pltpu.make_async_copy(span, span, sem).wait()

    idx_cp = pltpu.make_async_copy(idx_hbm, idx_v, lsem.at[0])
    idx_cp.start()
    barrier = pltpu.get_barrier_semaphore()
    for peer in (diag, up, down):
        pl.semaphore_signal(barrier, 1, device_id=(peer,), device_id_type=MESH)
    for c in range(AHEAD):
        x_copy(c).start()
    ebuf[...] = jnp.zeros(ebuf.shape, jnp.uint32)

    row = lax.broadcasted_iota(jnp.int32, (128, 128), 0)
    col = lax.broadcasted_iota(jnp.int32, (128, 128), 1)
    upper = jnp.where(row < col, 1.0, 0.0).astype(jnp.bfloat16)
    ones = jnp.ones((128, 128), jnp.bfloat16)
    lower = jnp.where((row > col) & (row // 8 == col // 8), 1.0, 0.0).astype(jnp.bfloat16)
    lane = lax.broadcasted_iota(jnp.int32, (8, 128), 1)

    def route(idx, seen):
        idx = jnp.where(idx < 0, idx + E, idx)
        hot = [idx == e for e in range(E)]
        rank = jnp.zeros((8, 128), jnp.float32)
        cum = jnp.zeros((8, 128), jnp.float32)
        total = []
        for g in range(E // 16):
            m = jnp.concatenate(
                [jnp.where(hot[g * 16 + k], 1.0, 0.0) for k in range(16)], axis=0
            ).astype(jnp.bfloat16)
            inrow = jnp.dot(m, upper, preferred_element_type=jnp.float32)
            rowtot = jnp.dot(m, ones, preferred_element_type=jnp.float32)
            above = jnp.dot(lower, rowtot.astype(jnp.bfloat16),
                            preferred_element_type=jnp.float32)
            for k in range(16):
                e, rows = g * 16 + k, slice(k * 8, (k + 1) * 8)
                before = above[rows] if seen is None else above[rows] + seen[e]
                incl = before + rowtot[rows]
                rank = jnp.where(hot[e], before + inrow[rows], rank)
                cum = jnp.where(lane == e, incl, cum)
                total.append(incl[7:])
        rank = rank.astype(jnp.int32)
        valid = (idx >= 0) & (idx < E) & (rank < CAP)
        return jnp.where(valid, idx * CAPP + rank, SPARE) * XR, cum.astype(jnp.int32), total

    def slot_copy(lo, hi, k):
        rows = pl.ds(lo, hi - lo)
        return pltpu.make_async_copy(slot_v.at[rows], slot_s.at[rows], lsem.at[k])

    idx_cp.wait()
    slot0, cum0, seen = route(idx_v[:8], None)
    slot_v[:8] = jnp.minimum(cum0, CAP) * XR
    slot_v[8:16] = slot0
    slot_copy(0, 16, 0).start()
    slot1, cum1, _ = route(idx_v[8:], seen)
    slot_v[16:] = slot1
    slot_copy(16, 24, 1).start()
    srow = lax.broadcasted_iota(jnp.int32, (8, 128), 0)
    cnt_all[me] = jnp.where(srow < 7, cum0, cum1)

    def first(src, own, j):
        return tab_s[src, own * EL + j]

    def kept(src, own, j):
        return tab_s[NDEV + src, own * EL + j]

    def hopped(src, own, j):
        return tab_s[2 * NDEV + src, own * EL + j]

    def positions():
        pltpu.make_async_copy(
            cnt_all.at[pl.ds(1, NDEV - 1)], cnt_all.at[pl.ds(1, NDEV - 1)], c_recv).wait()
        trow = lax.broadcasted_iota(jnp.int32, (16, 128), 0)
        tab = jnp.zeros((16, 128), jnp.int32)
        base = jnp.zeros((1, 128), jnp.int32)
        mine = jnp.zeros((1, 128), jnp.int32)
        for s in range(NDEV):
            cnt = cnt_all[s, 7:8, :]
            blind = jnp.minimum(cnt_all[s, BLIND * CR - 1:BLIND * CR, :], CAP)
            fit = jnp.clip(CAP - base, 0, cnt)
            mine = jnp.where(me == s, fit, mine)
            tab = jnp.where(trow == s, jnp.minimum(base, CAP), tab)
            tab = jnp.where(trow == NDEV + s, fit, tab)
            tab = jnp.where(trow == 2 * NDEV + s, jnp.maximum(fit, blind), tab)
            base = base + cnt
        tab_v[:16] = tab
        blind = jnp.minimum(cum0[BLIND * CR - 1:BLIND * CR], CAP)
        tab_v[16:24] = XR * jnp.maximum(jnp.minimum(cum0, mine), blind)
        tab_v[24:] = XR * jnp.maximum(jnp.minimum(cum1, mine), blind)
        tab_cp = pltpu.make_async_copy(tab_v, tab_s, lsem.at[0])
        tab_cp.start()
        tab_cp.wait()

    through = ((down, up, 0), (up, down, 1))

    def send_direct(j, lo, hi):
        for own in (up, down):
            e = own * EL + j
            r0, n = lo(e), hi(e) - lo(e)
            pl.when(n > 0)(remote(
                sbuf.at[pl.ds(e * (CAPP * XR) + r0, n)],
                ebuf.at[j, pl.ds(first(me, own, j) * XR + r0, n)],
                x_send, d_recv.at[j], own).start)

    def early_rows(e):
        return jnp.where(me == NDEV - 1,
                         jnp.minimum(tab_s[16 + (EARLY + 1) * CR - 1, e], tab_s[NDEV + me, e] * XR), 0)

    for c in range(NCH):
        x_copy(c).wait()
        if c + AHEAD < NCH:
            x_copy(c + AHEAD).start()
        if c == NCH - 1:
            for j in range(EL):
                w_copy(j).start()

        def pack_rows(b, _):
            r0 = pl.multiple_of(c * XCH + b * 64, 64)
            for q in range(XR):
                lo = xf[pl.ds(r0, 64), q * 128:(q + 1) * 128]
                hi = xf[pl.ds(r0, 64), (q + XR) * 128:(q + XR + 1) * 128]
                xp[pl.ds(r0 * XR + q, 64, stride=XR), :] = _pack(lo, hi)
        lax.fori_loop(0, XCH // 64, pack_rows, None)

        if c == 0:
            slot_copy(0, 16, 0).wait()
        if c == NCH // 2:
            slot_copy(16, 24, 1).wait()

        def sort_rows(b, _):
            r = c * (XCH // 128) + b
            for l in range(128):
                sbuf[pl.ds(slot_s[8 + r, l], XR), :] = xp[pl.ds((r * 128 + l) * XR, XR), :]
        lax.fori_loop(0, XCH // 128, sort_rows, None)

        if c == 0:
            pl.semaphore_wait(barrier, NDEV - 1)
            for peer in (diag, up, down):
                remote(cnt_all.at[me], cnt_all.at[me], x_send, c_recv, peer).start()
        if c == BLIND:
            positions()

        def rows_sent(k, e):
            if k < 0:
                return 0
            r = (k + 1) * CR - 1
            return slot_s[r, e] if k < BLIND else tab_s[16 + r, e]

        for j in range(EL):
            e = diag * EL + j
            lo = rows_sent(c - 1, e)
            n = rows_sent(c, e) - lo
            pl.when(n > 0)(remote(
                sbuf.at[pl.ds(e * (CAPP * XR) + lo, n)], xfwd.at[j, pl.ds(lo, n)],
                x_send, f_recv.at[j], (up, down)[j % 2]).start)

        if c == EARLY:
            @pl.when(me == NDEV - 1)
            def _():
                lax.fori_loop(
                    0, EL, lambda j, _: send_direct(j, lambda e: 0, early_rows), None)

    def x_src(own, j):
        return sbuf.at[pl.ds((own * EL + j) * (CAPP * XR), kept(me, own, j) * XR)]

    def x_dst(src, own, j):
        return ebuf.at[j, pl.ds(first(src, own, j) * XR, kept(src, own, j) * XR)]

    def send_rest(j):
        send_direct(j, early_rows, lambda e: tab_s[NDEV + me, e] * XR)

    send_rest(0)

    def forward_x(j, sent):
        pl.when(j + 1 < EL)(lambda: send_rest(jnp.minimum(j + 1, EL - 1)))
        origin = jnp.where(j % 2 == 0, down, up)
        target = jnp.where(j % 2 == 0, up, down)
        n = kept(origin, target, j)
        wait_rows(xfwd.at[j], hopped(origin, target, j) * XR, f_recv.at[j])
        pl.when(n > 0)(remote(
            xfwd.at[j, pl.ds(0, n * XR)], x_dst(origin, target, j),
            x_send, d_recv.at[j], target).start)
        return sent + XR * (n + kept(me, up, j) + kept(me, down, j) + hopped(me, diag, j))
    x_rows = lax.fori_loop(0, EL, forward_x, (NDEV - 1) * 8)

    def send_local(j, rows):
        pl.when(kept(me, me, j) > 0)(
            pltpu.make_async_copy(x_src(me, j), x_dst(me, me, j), lsem.at[0]).start)
        return rows + kept(me, me, j) * XR
    local_rows = lax.fori_loop(0, EL, send_local, 0)

    def tally(j, acc):
        return tuple(acc[i] + kept(i // NDEV, i % NDEV, 2 * j) for i in range(NDEV * NDEV)) + \
            tuple(acc[NDEV * NDEV + i] + kept(i // NDEV, i % NDEV, 2 * j + 1)
                  for i in range(NDEV * NDEV))
    acc = lax.fori_loop(0, EL // 2, tally, (0,) * (2 * NDEV * NDEV))
    even = lambda s, o: acc[s % NDEV * NDEV + o % NDEV]
    odd = lambda s, o: acc[NDEV * NDEV + s % NDEV * NDEV + o % NDEV]
    both = lambda s, o: even(s, o) + odd(s, o)
    lup = [XR * (both(s, s + 1) + even(s, s + 2) + even(s - 1, s + 1)) + YR * both(s + 1, s)
           for s in range(NDEV)]
    ldn = [XR * (both(s, s - 1) + odd(s, s + 2) + odd(s + 1, s - 1)) + YR * both(s - 1, s)
           for s in range(NDEV)]
    far = [YR * both(s + 2, s) for s in range(NDEV)]
    y3 = far[3] >> 1
    y0 = jnp.clip(((ldn[3] - lup[0] + far[0] + far[3] - BIAS_A) >> 1) - y3, 0, far[0])
    y2 = jnp.clip(((ldn[2] - lup[3] + far[2] + far[3] - BIAS_B) >> 1) - y3, 0, far[2])
    y1 = jnp.clip((ldn[1] - lup[1] + far[1] + far[2] - y2 - y0) >> 1, 0, far[1])
    for s, y in enumerate((y0, y1, y2, y3)):
        share = 0
        for bit in (256, 128, 64, 32, 16, 8, 4, 2, 1):
            share = jnp.where((share + bit) * far[s] <= y * 256, share + bit, share)
        share_s[s] = jnp.minimum(share, 256)

    def part(own, dst, j, side):
        n = kept(dst, own, j)
        cut = (n * share_s[own] + 128) >> 8
        return (0, cut) if side == 0 else (cut, n - cut)

    wait_rows(xp, local_rows, lsem.at[0])

    def y_src(dst, j):
        return ybuf.at[j, pl.ds(first(dst, me, j) * YR, kept(dst, me, j) * YR)]

    def y_dst(own, dst, j):
        return rbuf.at[pl.ds((own * EL + j) * (CAPP * YR), kept(dst, own, j) * YR)]

    def expert(j, sent):
        w_copy(j).wait()
        wait_rows(ebuf.at[j], XR * (kept(up, me, j) + kept(down, me, j)
                                    + kept(diag, me, j)), d_recv.at[j])
        a = [ebuf[j, pl.ds(q, CAPP, stride=XR), :] for q in range(XR)]
        lhs = jnp.concatenate(
            [_unpack(a[q], i).astype(jnp.bfloat16) for i in range(2) for q in range(XR)],
            axis=1)
        for q in range(YR):
            y = jnp.dot(lhs, wf[j, :, q * 256:(q + 1) * 256].astype(jnp.bfloat16),
                        preferred_element_type=jnp.float32)
            ybuf[j, pl.ds(q, CAPP, stride=YR), :] = _pack(y[:, :128], y[:, 128:])
        for side, mid in enumerate((up, down)):
            lo, n = part(me, diag, j, side)
            pl.when(n > 0)(remote(
                ybuf.at[j, pl.ds((first(diag, me, j) + lo) * YR, n * YR)],
                yfwd.at[side, j, pl.ds(0, n * YR)], y_send, g_recv.at[j // HALF], mid).start)
        for dst in (up, down):
            pl.when(kept(dst, me, j) > 0)(remote(
                y_src(dst, j), y_dst(me, dst, j), y_send, near_recv.at[j // HALF], dst).start)
        return sent + YR * (kept(diag, me, j) + kept(up, me, j) + kept(down, me, j))
    y_rows = lax.fori_loop(0, EL, expert, 0)

    out_ref[...] = jnp.zeros(out_ref.shape, jnp.float32)

    def invert(r, _):
        for l in range(128):
            inv_s[slot_s[8 + r, l] >> 1] = r * H + l // 8 * (H // 16) + l % 8

    def place(own, j, src, row0):
        n = kept(me, own, j)
        s0 = (own * EL + j) * CAPP

        def move(r):
            w = src[pl.ds(row0 + r * YR, YR), :]
            o = inv_s[s0 + r]
            for i in range(2):
                out_ref[pl.ds(o + 8 * i, YR, stride=16), :] = _unpack(w, i)

        def move8(b, _):
            for u in range(8):
                move(b * 8 + u)
        lax.fori_loop(0, n >> 3, move8, None)
        lax.fori_loop(n & ~7, n, lambda r, _: move(r), None)

    def forward_rows(j, rows):
        return rows + YR * sum(part(origin, target, j, side)[1]
                               for origin, target, side in through)

    def forward_y(j, _):
        for origin, target, side in through:
            lo, n = part(origin, target, j, side)
            pl.when(n > 0)(remote(
                yfwd.at[side, j, pl.ds(0, n * YR)],
                rbuf.at[pl.ds(((origin * EL + j) * CAPP + lo) * YR, n * YR)],
                y_send, diag_recv.at[j], target).start)

    def place_near(j, _):
        place(me, j, ybuf.at[j], first(me, me, j) * YR)
        for own in (up, down):
            place(own, j, rbuf, (own * EL + j) * (CAPP * YR))

    def near_rows(j, rows):
        return rows + YR * (kept(me, up, j) + kept(me, down, j))

    lax.fori_loop(0, TR, invert, None)

    def combine_half(h, sent):
        lo, hi = h * HALF, (h + 1) * HALF
        rows = lax.fori_loop(lo, hi, forward_rows, 0)
        wait_rows(xp, rows, g_recv.at[h])
        lax.fori_loop(lo, hi, forward_y, None)
        wait_rows(xp, lax.fori_loop(lo, hi, near_rows, 0), near_recv.at[h])
        lax.fori_loop(lo, hi, place_near, None)
        return sent + rows
    y_rows = lax.fori_loop(0, EL // HALF, combine_half, y_rows)

    wait_rows(sbuf, x_rows, x_send)

    def collect_diag(j, _):
        row0 = (diag * EL + j) * (CAPP * YR)
        wait_rows(rbuf.at[pl.ds(row0, CAPP * YR)], YR * kept(me, diag, j), diag_recv.at[j])
        place(diag, j, rbuf, row0)
    lax.fori_loop(0, EL, collect_diag, None)

    wait_rows(rbuf, y_rows, y_send)


def pallas_dist_moe_cap_ep_tokshard_n2048_d512_e8_h1024_kernel(
    x: jax.Array,
    router_W: jax.Array,
    route_idx: jax.Array,
    expert_W: jax.Array,
):
    del router_W
    u32, i32, f32 = jnp.uint32, jnp.int32, jnp.float32
    dma = pltpu.SemaphoreType.DMA
    out = pl.pallas_call(
        _body,
        out_shape=jax.ShapeDtypeStruct((T * H // 128, 128), f32),
        in_specs=[
            pl.BlockSpec(memory_space=pltpu.HBM),
            pl.BlockSpec(memory_space=pltpu.HBM),
            pl.BlockSpec(memory_space=pltpu.HBM),
        ],
        out_specs=pl.BlockSpec(memory_space=pltpu.VMEM),
        scratch_shapes=[
            pltpu.VMEM((T, D), f32),
            pltpu.VMEM((T * XR, 128), u32),
            pltpu.VMEM((SPARE * XR + 8, 128), u32),
            pltpu.VMEM((EL, CAPP * XR, 128), u32),
            pltpu.VMEM((EL, D, H), f32),
            pltpu.VMEM((EL, CAPP * YR, 128), u32),
            pltpu.VMEM((SPARE * YR, 128), u32),
            pltpu.VMEM((EL, CAPP * XR, 128), u32),
            pltpu.VMEM((2, EL, CAPP * YR, 128), u32),
            pltpu.VMEM((TR, 128), i32),
            pltpu.VMEM((NDEV, 8, 128), i32),
            pltpu.VMEM((TR + 8, 128), i32),
            pltpu.VMEM((32, 128), i32),
            pltpu.SMEM((TR + 8, 128), i32),
            pltpu.SMEM((32, 128), i32),
            pltpu.SMEM((SPARE + 8,), i32),
            pltpu.SMEM((NDEV,), i32),
            dma((max(NCH, EL),)), dma((2,)), dma, dma, dma,
            dma((EL,)), dma((EL,)), dma((2,)), dma((2,)), dma((EL,)),
        ],
        compiler_params=pltpu.CompilerParams(
            collective_id=0, vmem_limit_bytes=64 * 2**20),
    )(route_idx.reshape(TR, 128), x, expert_W)
    return out.reshape(T // 8, H // 128, 8, 128).transpose(0, 2, 1, 3).reshape(T, H)
```
